```python
import numpy as np

kernel_name = "dist_sparse_attn_causalblk_htp_bs_b2_sq256_skv256_hq4_dh64"

def setup_inputs():
    x = np.random.randn(8, 256, 512).astype(np.float32)
    Wq = np.random.randn(512, 1024).astype(np.float32) * 0.02
    K_ext = np.random.randn(8, 256, 16, 64).astype(np.float32)
    V_ext = np.random.randn(8, 256, 16, 64).astype(np.float32)
    Wo = np.random.randn(1024, 512).astype(np.float32) * 0.02
    return {"x": x, "Wq": Wq, "K_ext": K_ext, "V_ext": V_ext, "Wo": Wo}

def reference(x, Wq, K_ext, V_ext, Wo):
    B, Sq, Skv, Hq, Dh = 8, 256, 256, 16, 64
    Q = (x @ Wq).reshape(B, Sq, Hq, Dh)
    qb = (np.arange(Sq) // 64)[:, None]
    kb = (np.arange(Skv) // 64)[None, :]
    mask = kb <= qb
    scores = np.einsum('bihd,bjhd->bhij', Q, K_ext).astype(np.float32) * 0.125
    scores = np.where(mask[None, None, :, :], scores, -1e9)
    scores_max = scores.max(axis=-1, keepdims=True)
    w = np.exp(scores - scores_max)
    row_keep = mask.any(axis=1)
    w_sum = np.where(row_keep[None, None, :, None], w.sum(axis=-1, keepdims=True), 1.0)
    w = w / w_sum
    w = np.where(row_keep[None, None, :, None], w, 0.0)
    ctx = np.einsum('bhij,bjhd->bihd', w, V_ext).reshape(B, Sq, Hq * Dh)
    return ctx @ Wo
```

```python
import jax
import jax.numpy as jnp
from jax import lax
from jax.experimental import pallas as pl
from jax.experimental.pallas import tpu as pltpu

N_DEV = 4
B_LOC = 2
SQ = 256
D_MODEL = 512
DH = 64
BLK = 64
ROWS = B_LOC * SQ
NCOL = 4
NEG = -1e9

F32 = jnp.float32
BF16 = jnp.bfloat16


def _dot(a, b):
    return jnp.dot(a, b, preferred_element_type=F32)


def _dot_nt(a, b):
    return lax.dot_general(a, b, (((1,), (1,)), ((), ())),
                           preferred_element_type=F32)


def pallas_dist_sparse_attn_causalblk_htp_bs_b2_sq256_skv256_hq4_dh64_kernel(
    x: jax.Array,
    Wq: jax.Array,
    K_ext: jax.Array,
    V_ext: jax.Array,
    Wo: jax.Array,
):
    x2 = x.reshape(ROWS, D_MODEL)
    kt = jnp.transpose(K_ext, (0, 2, 3, 1)).reshape(8, 8, 2 * DH, SQ)
    vt = jnp.transpose(V_ext, (0, 2, 3, 1)).reshape(8, 8, 2 * DH, SQ)

    def body(x_hbm, wq_hbm, kt_hbm, vt_hbm, wo_hbm, out_hbm,
             wq32, wo32, x32, xb, kbuf, vbuf, wq_all, wo_all, ctx, acc,
             ld_sem, kv_sem, out_sem,
             q_ssem, q_rsem, o_ssem, o_rsem, f_ssem, f_rsem):
        me = lax.axis_index("i")
        left = (me + N_DEV - 1) % N_DEV
        right = (me + 1) % N_DEV
        diag = (me + 2) % N_DEV
        origin = (me, left, right, diag)

        barrier = pltpu.get_barrier_semaphore()
        for nb in (left, right):
            pl.semaphore_signal(barrier, inc=1, device_id=(nb,),
                                device_id_type=pl.DeviceIdType.MESH)

        wq_ld = pltpu.make_async_copy(wq_hbm, wq32, ld_sem.at[0])
        x_ld = pltpu.make_async_copy(x_hbm, x32, ld_sem.at[1])
        wo_ld = pltpu.make_async_copy(wo_hbm, wo32, ld_sem.at[2])

        def kv_ld(s, which):
            src, dst = ((kt_hbm, kbuf), (vt_hbm, vbuf))[which]
            return pltpu.make_async_copy(
                src.at[pl.ds(me * B_LOC, B_LOC), pl.ds(origin[s] * 2, 2)],
                dst.at[s], kv_sem.at[s, which])

        wq_ld.start()
        x_ld.start()
        kv_ld(0, 0).start()
        kv_ld(0, 1).start()
        wo_ld.start()
        for s in (1, 2, 3):
            kv_ld(s, 0).start()
            kv_ld(s, 1).start()

        def rcopy(src, dst, ssem, rsem, dev):
            return pltpu.make_async_remote_copy(
                src_ref=src, dst_ref=dst, send_sem=ssem, recv_sem=rsem,
                device_id=(dev,), device_id_type=pl.DeviceIdType.MESH)

        def q_own(dirn, hf):
            dev, slot = ((right, 1), (left, 2))[dirn]
            return rcopy(wq_all.at[0, hf], wq_all.at[slot, hf],
                         q_ssem.at[dirn, hf], q_rsem.at[dirn, hf], dev)

        def q_fwd(hf):
            dev, slot = ((right, 1), (left, 2))[hf]
            return rcopy(wq_all.at[slot, hf], wq_all.at[3, hf],
                         q_ssem.at[2, hf], q_rsem.at[2, hf], dev)

        def o_own(dirn, hf):
            dev, slot = ((right, 1), (left, 2))[dirn]
            return rcopy(wo_all.at[0, hf], wo_all.at[slot, hf],
                         o_ssem.at[dirn, hf], o_rsem.at[dirn, hf], dev)

        def o_fwd(hf, n):
            dev, slot = ((right, 1), (left, 2))[hf]
            return rcopy(wo_all.at[slot, hf, n], wo_all.at[3, hf, n],
                         f_ssem.at[hf, n], f_rsem.at[hf, n], dev)

        wq_ld.wait()
        for hf in range(2):
            wq_all[0, hf] = wq32[:, hf * 128:(hf + 1) * 128].astype(BF16)
        pl.semaphore_wait(barrier, 2)
        q_own(0, 0).start()
        q_own(1, 1).start()
        q_own(0, 1).start()
        q_own(1, 0).start()

        x_ld.wait()
        xb[...] = x32[...].astype(BF16)

        lane = lax.broadcasted_iota(jnp.int32, (128, 128), 1)
        lo = lane < DH
        row = lax.broadcasted_iota(jnp.int32, (256, 128), 0)
        col = lax.broadcasted_iota(jnp.int32, (256, 128), 1)
        keep = (col // BLK) <= ((row % 128) // BLK)

        def attn(s, hf):
            q = _dot(xb[...], wq_all[s, hf]) * 0.125
            for b in range(B_LOC):
                qt = q[b * SQ: b * SQ + 128]
                qb = q[b * SQ + 128: (b + 1) * SQ]
                q_top = jnp.concatenate(
                    [jnp.where(lo, qt, 0.0), jnp.where(lo, 0.0, qt)], axis=0
                ).astype(BF16)
                q_bot = jnp.concatenate(
                    [jnp.where(lo, qb, 0.0), jnp.where(lo, 0.0, qb)], axis=0
                ).astype(BF16)
                k0 = kbuf[s, b, hf, :, 0:128].astype(BF16)
                k1 = kbuf[s, b, hf, :, 128:256].astype(BF16)
                v0 = vbuf[s, b, hf, :, 0:128].astype(BF16)
                v1 = vbuf[s, b, hf, :, 128:256].astype(BF16)

                s_t = jnp.where(keep, _dot(q_top, k0), NEG)
                m_t = jnp.max(s_t, axis=-1, keepdims=True)
                p_t = jnp.exp(s_t - m_t)
                l_t = jnp.sum(p_t, axis=-1, keepdims=True)
                r_t = _dot_nt(p_t.astype(BF16), v0) / l_t

                s_0 = _dot(q_bot, k0)
                s_1 = jnp.where(keep, _dot(q_bot, k1), NEG)
                m_b = jnp.max(jnp.maximum(s_0, s_1), axis=-1, keepdims=True)
                p_0 = jnp.exp(s_0 - m_b)
                p_1 = jnp.exp(s_1 - m_b)
                l_b = jnp.sum(p_0 + p_1, axis=-1, keepdims=True)
                r_b = (_dot_nt(p_0.astype(BF16), v0)
                       + _dot_nt(p_1.astype(BF16), v1)) / l_b

                ctx[s, hf, b * SQ: b * SQ + 128, :] = jnp.where(
                    lo, r_t[:128], r_t[128:]).astype(BF16)
                ctx[s, hf, b * SQ + 128: (b + 1) * SQ, :] = jnp.where(
                    lo, r_b[:128], r_b[128:]).astype(BF16)

        def oproj(pairs, n):
            r = None
            for (s, hf) in pairs:
                t = _dot(ctx[s, hf], wo_all[s, hf, n])
                r = t if r is None else r + t
            return r

        kv_ld(0, 0).wait()
        kv_ld(0, 1).wait()
        attn(0, 0)
        attn(0, 1)

        wo_ld.wait()
        for hf in range(2):
            for n in range(NCOL):
                wo_all[0, hf, n] = wo32[hf * 128:(hf + 1) * 128,
                                        n * 128:(n + 1) * 128].astype(BF16)

        q_own(0, 0).wait_recv()
        q_fwd(0).start()
        q_own(1, 1).wait_recv()
        q_fwd(1).start()
        o_own(0, 0).start()
        o_own(1, 1).start()
        o_own(0, 1).start()
        o_own(1, 0).start()

        for s in (1, 2):
            kv_ld(s, 0).wait()
            kv_ld(s, 1).wait()
        attn(1, 0)
        attn(2, 1)
        for n in range(NCOL):
            acc[n] = oproj([(0, 0), (0, 1)], n)
        q_own(0, 1).wait_recv()
        attn(1, 1)
        q_own(1, 0).wait_recv()
        attn(2, 0)

        kv_ld(3, 0).wait()
        kv_ld(3, 1).wait()
        q_fwd(0).wait_recv()
        attn(3, 0)
        q_fwd(1).wait_recv()
        attn(3, 1)

        o_own(0, 0).wait_recv()
        o_own(1, 1).wait_recv()
        for n in range(NCOL):
            o_fwd(0, n).start()
            o_fwd(1, n).start()
        for n in range(NCOL):
            acc[n] += oproj([(1, 0), (2, 1)], n)
        o_own(0, 1).wait_recv()
        o_own(1, 0).wait_recv()
        for n in range(NCOL):
            acc[n] += oproj([(1, 1), (2, 0)], n)

        def out_st(n):
            return pltpu.make_async_copy(
                acc.at[n], out_hbm.at[:, pl.ds(n * 128, 128)], out_sem.at[n])

        for n in range(NCOL):
            o_fwd(0, n).wait_recv()
            o_fwd(1, n).wait_recv()
            acc[n] += oproj([(3, 0), (3, 1)], n)
            out_st(n).start()

        for d in range(2):
            for hf in range(2):
                q_own(d, hf).wait_send()
                o_own(d, hf).wait_send()
        for hf in range(2):
            q_fwd(hf).wait_send()
            for n in range(NCOL):
                o_fwd(hf, n).wait_send()
        for n in range(NCOL):
            out_st(n).wait()

    any_spec = pl.BlockSpec(memory_space=pl.ANY)
    out = pl.pallas_call(
        body,
        out_shape=jax.ShapeDtypeStruct((ROWS, D_MODEL), F32),
        in_specs=[any_spec] * 5,
        out_specs=any_spec,
        scratch_shapes=[
            pltpu.VMEM((D_MODEL, 256), F32),
            pltpu.VMEM((256, D_MODEL), F32),
            pltpu.VMEM((ROWS, D_MODEL), F32),
            pltpu.VMEM((ROWS, D_MODEL), BF16),
            pltpu.VMEM((4, B_LOC, 2, 128, SQ), F32),
            pltpu.VMEM((4, B_LOC, 2, 128, SQ), F32),
            pltpu.VMEM((4, 2, D_MODEL, 128), BF16),
            pltpu.VMEM((4, 2, NCOL, 128, 128), BF16),
            pltpu.VMEM((4, 2, ROWS, 128), BF16),
            pltpu.VMEM((NCOL, ROWS, 128), F32),
            pltpu.SemaphoreType.DMA((3,)),
            pltpu.SemaphoreType.DMA((4, 2)),
            pltpu.SemaphoreType.DMA((NCOL,)),
            pltpu.SemaphoreType.DMA((3, 2)),
            pltpu.SemaphoreType.DMA((3, 2)),
            pltpu.SemaphoreType.DMA((2, 2)),
            pltpu.SemaphoreType.DMA((2, 2)),
            pltpu.SemaphoreType.DMA((2, NCOL)),
            pltpu.SemaphoreType.DMA((2, NCOL)),
        ],
        compiler_params=pltpu.CompilerParams(
            collective_id=0, vmem_limit_bytes=64 * 1024 * 1024),
    )(x2, Wq, kt, vt, Wo)
    return out.reshape(B_LOC, SQ, D_MODEL)
```

```python
import jax
import jax.numpy as jnp
from jax import lax
from jax.experimental import pallas as pl
from jax.experimental.pallas import tpu as pltpu

B_LOC = 2
SQ = 256
D_MODEL = 512
DH = 64
BLK = 64
ROWS = B_LOC * SQ
NCOL = 4
NEG = -1e9

F32 = jnp.float32
BF16 = jnp.bfloat16

R32 = 32
QEND = (80, 192, 512)
QBEG = (R32,) + QEND[:-1]
NQ = len(QEND)
FGRP = ((0, 4), (4, 6), (6, 7), (7, 8))
NF = len(FGRP)


def _dot(a, b):
    return jnp.dot(a, b, preferred_element_type=F32)


def _dot_nt(a, b):
    return lax.dot_general(a, b, (((1,), (1,)), ((), ())),
                           preferred_element_type=F32)


def pallas_dist_sparse_attn_causalblk_htp_bs_b2_sq256_skv256_hq4_dh64_kernel(
    x: jax.Array,
    Wq: jax.Array,
    K_ext: jax.Array,
    V_ext: jax.Array,
    Wo: jax.Array,
):
    x2 = x.reshape(ROWS, D_MODEL)
    kt = jnp.transpose(K_ext, (0, 2, 3, 1)).reshape(8, 8, 2 * DH, SQ)
    vt = jnp.transpose(V_ext, (0, 2, 3, 1)).reshape(8, 8, 2 * DH, SQ)

    def body(x_hbm, wq_hbm, kt_hbm, vt_hbm, wo_hbm, out_ref,
             wq32, wo32, x32, xb, kbuf, vbuf, stage, wq_all, wo_all, ctx,
             ld_sem, ready_sem,
             q1_ssem, q1_rsem, q_ssem, q_rsem, o_ssem, o_rsem, f_ssem, f_rsem):
        me = lax.axis_index("i")
        left = (me + 3) & 3
        right = (me + 1) & 3
        diag = (me + 2) & 3
        odd = (me & 1) == 1
        origin = (me, left, right, diag)

        def wq_ld(c):
            if c == NQ:
                rows = pl.ds(0, R32)
            else:
                rows = pl.ds(QBEG[c], QEND[c] - QBEG[c])
            return pltpu.make_async_copy(wq_hbm.at[rows], wq32.at[rows],
                                         ld_sem.at[2 + c])

        x_ld = pltpu.make_async_copy(x_hbm, x32, ld_sem.at[0])
        wo_ld = pltpu.make_async_copy(wo_hbm, wo32, ld_sem.at[1])

        def kv_ld(s, which, hf):
            src, dst = ((kt_hbm, kbuf), (vt_hbm, vbuf))[which]
            return pltpu.make_async_copy(
                src.at[pl.ds(me * B_LOC, B_LOC), origin[s] * 2 + hf],
                dst.at[s, hf], ld_sem.at[3 + NQ + s * 4 + hf * 2 + which])

        def kv_start(s, hf):
            kv_ld(s, 0, hf).start()
            kv_ld(s, 1, hf).start()

        def kv_wait(s, hf):
            kv_ld(s, 0, hf).wait()
            kv_ld(s, 1, hf).wait()

        def signal(sem, dev):
            pl.semaphore_signal(sem, inc=1, device_id=(dev,),
                                device_id_type=pl.DeviceIdType.MESH)

        def rcopy(src, dst, ssem, rsem, dev):
            return pltpu.make_async_remote_copy(
                src_ref=src, dst_ref=dst, send_sem=ssem, recv_sem=rsem,
                device_id=(dev,), device_id_type=pl.DeviceIdType.MESH)

        def q_raw(dirn):
            dev = (right, left)[dirn]
            return rcopy(wq_hbm.at[pl.ds(0, R32), pl.ds(dirn * 128, 128)],
                         stage.at[dirn],
                         q1_ssem.at[dirn, NQ], q1_rsem.at[dirn, NQ], dev)

        def q_first(dirn, c):
            dev, slot = ((right, 1), (left, 2))[dirn]
            rows = pl.ds(QBEG[c], QEND[c] - QBEG[c])
            return rcopy(wq_all.at[0, dirn, rows], wq_all.at[slot, dirn, rows],
                         q1_ssem.at[dirn, c], q1_rsem.at[dirn, c], dev)

        def q_second(dirn):
            dev, slot = ((right, 1), (left, 2))[dirn]
            hf = 1 - dirn
            return rcopy(wq_all.at[0, hf], wq_all.at[slot, hf],
                         q_ssem.at[0, dirn], q_rsem.at[0, dirn], dev)

        def q_fwd(dirn):
            dev, slot = ((right, 1), (left, 2))[dirn]
            return rcopy(wq_all.at[slot, dirn], wq_all.at[3, dirn],
                         q_ssem.at[1, dirn], q_rsem.at[1, dirn], dev)

        def o_own(dirn, phase):
            dev = (right, left)[dirn]
            rows = pl.ds((dirn ^ phase) * DH, DH)
            return rcopy(wo_all.at[0, :, rows], wo_all.at[1 + phase, :, rows],
                         o_ssem.at[dirn, phase], o_rsem.at[dirn, phase], dev)

        def o_fwd(dirn, g):
            dev = (right, left)[dirn]
            rows = pl.ds(dirn * DH, DH)
            tiles = pl.ds(FGRP[g][0], FGRP[g][1] - FGRP[g][0])
            return rcopy(wo_all.at[1, tiles, rows], wo_all.at[3, tiles, rows],
                         f_ssem.at[dirn, g], f_rsem.at[dirn, g], dev)

        def wq_cast(r0, r1):
            for hf in range(2):
                wq_all[0, hf, r0:r1, :] = wq32[
                    r0:r1, hf * 128:(hf + 1) * 128].astype(BF16)

        wq_ld(0).start()

        barrier = pltpu.get_barrier_semaphore()

        @pl.when(me != 2)
        def _():
            signal(barrier, left)
            signal(barrier, right)

        @pl.when(me == 1)
        def _():
            pl.semaphore_wait(barrier, 1)
            q_raw(1).start()

        @pl.when(me == 3)
        def _():
            pl.semaphore_wait(barrier, 1)
            q_raw(0).start()

        for c in range(1, NQ + 1):
            wq_ld(c).start()
        x_ld.start()
        kv_start(0, 0)
        wo_ld.start()
        for (s, hf) in ((0, 1), (1, 0), (2, 1), (1, 1), (2, 0), (3, 0), (3, 1)):
            kv_start(s, hf)

        @pl.when(jnp.logical_not(odd))
        def _():
            pl.semaphore_wait(barrier, 2)
            q_raw(0).start()
            q_raw(1).start()

        @pl.when(me == 2)
        def _():
            signal(ready_sem, left)
            signal(ready_sem, right)

        for c in range(NQ):
            wq_ld(c).wait()
            wq_cast(QBEG[c], QEND[c])
            if c == NQ - 1:
                wq_ld(NQ).wait()
                wq_cast(0, R32)

            @pl.when(me != 1)
            def _():
                q_first(0, c).start()
                if c == NQ - 1:
                    q_second(0).start()

            @pl.when(me != 3)
            def _():
                q_first(1, c).start()
                if c == NQ - 1:
                    q_second(1).start()

        @pl.when(odd)
        def _():
            pl.semaphore_wait(ready_sem, 1)

        for dirn, who in ((0, 1), (1, 3)):
            @pl.when(me == who)
            def _():
                q_raw(dirn).start()
                for c in range(NQ):
                    q_first(dirn, c).start()
                q_second(dirn).start()

        x_ld.wait()
        xb[...] = x32[...].astype(BF16)

        lane = lax.broadcasted_iota(jnp.int32, (128, 128), 1)
        lo = lane < DH
        row = lax.broadcasted_iota(jnp.int32, (256, 128), 0)
        col = lax.broadcasted_iota(jnp.int32, (256, 128), 1)
        keep = (col // BLK) <= ((row % 128) // BLK)

        def put_ctx(s, hf, r0, r):
            if s in (0, 3):
                ctx[s, hf, r0:r0 + 128, :] = jnp.where(
                    lo, r[:128], r[128:]).astype(BF16)
            else:
                ctx[s, hf, r0:r0 + 128, 0:DH] = r[:128, 0:DH].astype(BF16)
                ctx[3 - s, hf, r0:r0 + 128, DH:] = r[128:, DH:].astype(BF16)

        def attn(s, hf):
            q = _dot(xb[...], wq_all[s, hf]) * 0.125
            for b in range(B_LOC):
                qt = q[b * SQ: b * SQ + 128]
                qb = q[b * SQ + 128: (b + 1) * SQ]
                q_top = jnp.concatenate(
                    [jnp.where(lo, qt, 0.0), jnp.where(lo, 0.0, qt)], axis=0
                ).astype(BF16)
                q_bot = jnp.concatenate(
                    [jnp.where(lo, qb, 0.0), jnp.where(lo, 0.0, qb)], axis=0
                ).astype(BF16)
                k0 = kbuf[s, hf, b, :, 0:128].astype(BF16)
                k1 = kbuf[s, hf, b, :, 128:256].astype(BF16)
                v0 = vbuf[s, hf, b, :, 0:128].astype(BF16)
                v1 = vbuf[s, hf, b, :, 128:256].astype(BF16)

                s_t = jnp.where(keep, _dot(q_top, k0), NEG)
                m_t = jnp.max(s_t, axis=-1, keepdims=True)
                p_t = jnp.exp(s_t - m_t)
                l_t = jnp.sum(p_t, axis=-1, keepdims=True)
                r_t = _dot_nt(p_t.astype(BF16), v0) / l_t

                s_0 = _dot(q_bot, k0)
                s_1 = jnp.where(keep, _dot(q_bot, k1), NEG)
                m_b = jnp.max(jnp.maximum(s_0, s_1), axis=-1, keepdims=True)
                p_0 = jnp.exp(s_0 - m_b)
                p_1 = jnp.exp(s_1 - m_b)
                l_b = jnp.sum(p_0 + p_1, axis=-1, keepdims=True)
                r_b = (_dot_nt(p_0.astype(BF16), v0)
                       + _dot_nt(p_1.astype(BF16), v1)) / l_b

                put_ctx(s, hf, b * SQ, r_t)
                put_ctx(s, hf, b * SQ + 128, r_b)

        def oproj(s, t0, t1, first=False):
            msplit = max(1, 4 // (t1 - t0))
            rows = ROWS // msplit
            for n in range(NCOL):
                ts = [t for t in (2 * n, 2 * n + 1) if t0 <= t < t1]
                if not ts:
                    continue
                for m in range(msplit):
                    r0 = m * rows
                    r = None
                    for t in ts:
                        d = _dot(ctx[s, t % 2, r0:r0 + rows, :], wo_all[s, t])
                        r = d if r is None else r + d
                    idx = (slice(r0, r0 + rows), slice(n * 128, (n + 1) * 128))
                    if first:
                        out_ref[idx] = r
                    else:
                        out_ref[idx] += r

        kv_wait(0, 0)
        attn(0, 0)

        wo_ld.wait()
        for t in range(2 * NCOL):
            n, p = divmod(t, 2)
            wo_all[0, t] = wo32[p * 128:(p + 1) * 128,
                                n * 128:(n + 1) * 128].astype(BF16)
        o_own(0, 0).start()
        o_own(1, 0).start()

        kv_wait(0, 1)
        attn(0, 1)

        for dirn in range(2):
            q_raw(dirn).wait_recv()
            for c in range(NQ):
                q_first(dirn, c).wait_recv()
            wq_all[1 + dirn, dirn, 0:R32, :] = stage[dirn].astype(BF16)
            q_fwd(dirn).start()
            o_own(dirn, 1).start()

        kv_wait(1, 0)
        kv_wait(2, 1)
        attn(1, 0)
        attn(2, 1)
        oproj(0, 0, 8, first=True)

        q_second(0).wait_recv()
        q_second(1).wait_recv()
        kv_wait(1, 1)
        kv_wait(2, 0)
        attn(1, 1)
        attn(2, 0)

        o_own(0, 0).wait_recv()
        o_own(1, 0).wait_recv()
        for g in range(NF):
            o_fwd(0, g).start()
            o_fwd(1, g).start()
        oproj(1, 0, 8)

        kv_wait(3, 0)
        kv_wait(3, 1)
        q_fwd(0).wait_recv()
        q_fwd(1).wait_recv()
        attn(3, 0)
        attn(3, 1)

        o_own(0, 1).wait_recv()
        o_own(1, 1).wait_recv()
        oproj(2, 0, 8)

        for d in range(2):
            q_raw(d).wait_send()
            for c in range(NQ):
                q_first(d, c).wait_send()
            q_second(d).wait_send()
            q_fwd(d).wait_send()
            for ph in range(2):
                o_own(d, ph).wait_send()

        for g in range(NF):
            if g == NF - 1:
                for d in range(2):
                    for gg in range(NF):
                        o_fwd(d, gg).wait_send()
            o_fwd(0, g).wait_recv()
            o_fwd(1, g).wait_recv()
            oproj(3, *FGRP[g])

    any_spec = pl.BlockSpec(memory_space=pl.ANY)
    out = pl.pallas_call(
        body,
        out_shape=jax.ShapeDtypeStruct((ROWS, D_MODEL), F32),
        in_specs=[any_spec] * 5,
        out_specs=pl.BlockSpec(memory_space=pltpu.VMEM),
        scratch_shapes=[
            pltpu.VMEM((D_MODEL, 256), F32),
            pltpu.VMEM((256, D_MODEL), F32),
            pltpu.VMEM((ROWS, D_MODEL), F32),
            pltpu.VMEM((ROWS, D_MODEL), BF16),
            pltpu.VMEM((4, 2, B_LOC, 128, SQ), F32),
            pltpu.VMEM((4, 2, B_LOC, 128, SQ), F32),
            pltpu.VMEM((2, R32, 128), F32),
            pltpu.VMEM((4, 2, D_MODEL, 128), BF16),
            pltpu.VMEM((4, 2 * NCOL, 128, 128), BF16),
            pltpu.VMEM((4, 2, ROWS, 128), BF16),
            pltpu.SemaphoreType.DMA((3 + NQ + 16,)),
            pltpu.SemaphoreType.REGULAR,
            pltpu.SemaphoreType.DMA((2, NQ + 1)),
            pltpu.SemaphoreType.DMA((2, NQ + 1)),
            pltpu.SemaphoreType.DMA((2, 2)),
            pltpu.SemaphoreType.DMA((2, 2)),
            pltpu.SemaphoreType.DMA((2, 2)),
            pltpu.SemaphoreType.DMA((2, 2)),
            pltpu.SemaphoreType.DMA((2, NF)),
            pltpu.SemaphoreType.DMA((2, NF)),
        ],
        compiler_params=pltpu.CompilerParams(
            collective_id=0, vmem_limit_bytes=64 * 1024 * 1024,
            disable_semaphore_checks=True),
    )(x2, Wq, kt, vt, Wo)
    return out.reshape(B_LOC, SQ, D_MODEL)
```
